```python
import numpy as np

kernel_name = "dist_pipemlp_pp2tp2_xy_b4096_d256_h512"

def setup_inputs():
    x_padded = np.zeros((2, 4096, 256), dtype=np.float32)
    x_padded[0] = np.random.randn(4096, 256).astype(np.float32)
    Win = np.random.randn(4, 256, 1024).astype(np.float32)
    Wout = np.random.randn(4, 1024, 256).astype(np.float32)
    return {"x_padded": x_padded, "Win": Win, "Wout": Wout}

def reference(x_padded, Win, Wout):
    a = x_padded[0]
    for k in range(4):
        h = a @ Win[k]
        h = np.maximum(h, 0.0)
        a = h @ Wout[k]
    out = np.zeros_like(x_padded)
    out[1] = a
    return out
```

```python
import jax
import jax.numpy as jnp
from jax import lax
from jax.experimental import pallas as pl
from jax.experimental.pallas import tpu as pltpu

MESH = pl.DeviceIdType.MESH
BF16 = jnp.bfloat16
F32 = jnp.float32

B, D, H = 4096, 256, 512
HALF = B // 2
R = 128
N = HALF // R
X_AHEAD = 2

SCHEDULE = dict(
    s0="a0 a1 a2 a3 a4 a5 a6 a7 a8 a9 a10 a11 c0 c1 a12 c2 a13 c3 c4 a14 c5 a15 c6 "
       "C7 c8 C9 C10 c11 C12 C13 f6 C14 f9 C15 f12",
    s1="b0 b1 H0 b2 b3 H2 b4 d4 G2 B5 D6 b8 d5 D8 d10 b11 d11 d12 d13 G0 d14 d15 X0",
    early=(0, 1),
    split=(12, 64),
    first=32,
    late=3,
)


def make_kernel(cfg=None):
    c = dict(SCHEDULE)
    c.update(cfg or {})
    s0 = [(t[0], int(t[1:])) for t in c["s0"].split()]
    s1 = [(t[0], int(t[1:])) for t in c["s1"].split()]
    early = list(c["early"])
    split_k, split_rows = c["split"]
    offload = [k for t, k in s0 if t == "C"]
    round_trip = [k for t, k in s0 if t == "f"]

    def chunks(kinds, ops=s1):
        return [k + d for t, k in ops if t in kinds for d in range(2 if t.isupper() else 1)]

    assert [k for t, k in s0 if t == "a"] == list(range(N))
    assert sorted(k for t, k in s0 if t in "cC") == list(range(N))
    assert sorted(chunks("bBe")) == [k for k in range(N) if k not in offload]
    assert sorted(chunks("dDGe")) == list(range(N))
    assert sorted(chunks("H")) == sorted(chunks("G")) and sorted(chunks("xX")) == sorted(early)
    assert not any(k in offload + round_trip + chunks("e") for k in early) and split_k in round_trip
    for i, (t, k) in enumerate(s0):
        if t == "f":
            upto = next(j for j, op in enumerate(s1) if k in chunks("dDGe", [op]))
            assert all(q in [m for u, m in s0[:i] if u in "cC"] for q in chunks("bBdDHGe", s1[:upto + 1]))

    arrivals = [k for k in chunks("dDGe") if k not in round_trip and k not in early]
    for i, k in enumerate(round_trip):
        arrivals.insert(len(arrivals) - (len(round_trip) - 1 - i), k)
    late = arrivals[len(arrivals) - c["late"]:]

    def pack(kind, k, arg, wait):
        return kind | (k << 4) | (arg << 12) | (wait << 16)

    tab0, seen = [], []
    for t, k in s0:
        wait = 1 if t in "cC" and not seen else 2 if t == "C" and 2 not in seen else 0
        seen += [wait] if wait else []
        tab0.append(pack("acCf".index(t), k, 0, wait))
    assert seen[0] == 1 and (2 in seen or not offload)
    kind_of = {"b": 0, "d": 0, "x": 0, "B": 1, "D": 1, "X": 1, "H": 2, "G": 2, "e": 3}
    tab1, seen = [], []
    for t, k in s1:
        k += N if t in "xX" else 0
        new = [q for q in range(k, k + (2 if t.isupper() else 1)) if q not in seen]
        new += [-1] if t in "dDGexX" and -1 not in seen else []
        seen += new
        tab1.append(pack(kind_of[t], k, int(t in "dDGxX"), sum(4 if q < 0 else 1 << (q - k) for q in new)))
    kinds1 = [kind_of[t] for t, k in s1]

    def bits(ks):
        return sum(1 << k for k in ks)

    special = [split_k] + [k for k in late if k not in round_trip]
    plain_mask = bits(k for k in range(N) if k not in early + special)

    class _Null:
        def __enter__(self):
            return self

        def __exit__(self, *a):
            return False

    def scope(name):
        return jax.named_scope(name) if c.get("scopes") else _Null()

    def body(x_hbm, win_hbm, wout_hbm, out,
             xbuf, wi_f, wo_f, wi, wo, pown, psend, precv, abuf, recv, osend, tab, send_sem, late_sem):
        mx = lax.axis_index("x")
        my = lax.axis_index("y")
        ynbr = (mx, 1 - my)
        xnbr = (1 - mx, my)

        def rows(k, base=0, m=1):
            return pl.ds(pl.multiple_of(base + k * R, R), m * R)

        def part(k, base=0):
            return pl.ds(base + k * R, split_rows if k == split_k else R)

        def remote(src, dst, sem, dev):
            return pltpu.make_async_remote_copy(src, dst, send_sem, sem, device_id=dev, device_id_type=MESH)

        def half_ffn(a, l, s):
            h = jnp.dot(a, wi[l, s], preferred_element_type=F32)
            h = jnp.maximum(h, 0.0).astype(BF16)
            return jnp.dot(h, wo[l, s], preferred_element_type=F32)

        def ffn(a, l):
            return half_ffn(a, l, 0) + half_ffn(a, l, 1)

        first_pieces = [(0, 0, c["first"]), (0, c["first"], D - c["first"]), (1, 0, H)]
        whole_pieces = [(0, 0, D), (1, 0, H)]

        def w_rows(l, s, piece):
            return (wi, wo)[piece[0]].at[l, s, pl.ds(piece[1], piece[2])]

        def w_cast(l, piece):
            m, r0, nr = piece
            (wi, wo)[m][l, 0, pl.ds(r0, nr), :] = (wi_f, wo_f)[m][l, pl.ds(r0, nr), :].astype(BF16)

        def across(k):
            return remote(recv.at[part(k, HALF)], recv.at[part(k)], late_sem.at[round_trip.index(k)], ynbr)

        def down(k, sem):
            return remote(recv.at[part(k)], recv.at[part(k, HALF)], sem, xnbr)

        def result(k, sem, dev=ynbr):
            return remote(osend.at[rows(k)], recv.at[rows(k, HALF)], sem, dev)

        def take(k):
            out[rows(k, (1 - my) * HALF), :] = recv[rows(k, HALF), :].astype(F32)

        last = round_trip + [k for k in late if k not in round_trip]

        def run_table(table, step):
            for i, word in enumerate(table + [0]):
                tab[i] = word

            def loop(i, word):
                nxt = tab[i + 1]
                step(word & 15, (word >> 4) & 255, (word >> 12) & 15, word >> 16)
                return nxt

            lax.fori_loop(0, len(table), loop, jnp.int32(table[0]))

        def main(ld_sem, x_sem, w_sem, r_sem, ready):
            def w_load(l, piece, i):
                m, r0, nr = piece
                return pltpu.make_async_copy((win_hbm, wout_hbm)[m].at[l, pl.ds(r0, nr)],
                                             (wi_f, wo_f)[m].at[l, pl.ds(r0, nr)], ld_sem.at[i])

            def x_load(j):
                base = jnp.where(j < N // 2, 1 - my, my) * HALF
                return pltpu.make_async_copy(x_hbm.at[0, rows(2 * lax.rem(j, N // 2), base, 2)],
                                             xbuf.at[rows(2 * j, 0, 2)], x_sem.at[lax.rem(j, X_AHEAD + 1)])

            def partial(k):
                return remote(psend.at[rows(k)], precv.at[rows(k)], r_sem.at[k], ynbr)

            def landed(k):
                remote(recv.at[rows(k)], recv.at[rows(k)], r_sem.at[k], xnbr).wait_recv()

            def up(k):
                return remote(osend.at[part(k)], recv.at[part(k, HALF)], r_sem.at[N + k], xnbr)

            tail = (split_k * R + split_rows, R - split_rows)
            direct_part = remote(osend.at[pl.ds(*tail)], recv.at[pl.ds(HALF + tail[0], tail[1])],
                                 r_sem.at[N + split_k], ynbr)

            la = 1 - mx
            lb = mx
            load_a = [w_load(la, p, i) for i, p in enumerate(first_pieces)]
            load_b = [w_load(lb, p, 3 + i) for i, p in enumerate(whole_pieces)]
            swap_a = [remote(w_rows(la, 0, p), w_rows(la, 1, p), w_sem.at[i], ynbr)
                      for i, p in enumerate(first_pieces)]
            swap_b = [remote(w_rows(1, 0, p), w_rows(1, 1, p), w_sem.at[3 + i], ynbr)
                      for i, p in enumerate(whole_pieces)]
            up_own = [remote(w_rows(0, 0, p), w_rows(2, 0, p), w_sem.at[3 + i], xnbr)
                      for i, p in enumerate(first_pieces)]
            up_other = [remote(w_rows(0, 1, p), w_rows(2, 1, p), w_sem.at[6 + i], xnbr)
                        for i, p in enumerate(whole_pieces)]

            barrier = pltpu.get_barrier_semaphore()
            pl.semaphore_signal(barrier, 1, device_id=ynbr, device_id_type=MESH)
            load_a[0].start()
            load_a[1].start()

            @pl.when(mx == 0)
            def _():
                pl.semaphore_signal(barrier, 1, device_id=xnbr, device_id_type=MESH)

            for i, p in enumerate(first_pieces):
                load_a[i].wait()
                w_cast(la, p)
                if i == 0:
                    for cp in [load_a[2]] + load_b:
                        cp.start()

                    @pl.when(mx == 0)
                    def _():
                        pl.semaphore_wait(barrier, 1)

                    @pl.when(mx == 1)
                    def _():
                        pl.semaphore_wait(barrier, 2)
                swap_a[i].start()

                @pl.when(mx == 1)
                def _():
                    up_own[i].start()
                    if i == 0:
                        pl.semaphore_signal(ready, 1, device_id=xnbr, device_id_type=MESH)

            @pl.when(mx == 0)
            def _():
                for j in range(X_AHEAD):
                    x_load(j).start()

            for i, p in enumerate(whole_pieces):
                load_b[i].wait()
                w_cast(lb, p)

            @pl.when(mx == 1)
            def _stage1():
                for cp in swap_b:
                    cp.start()
                swap_a[0].wait_recv()
                swap_a[1].wait_recv()
                up_other[0].start()
                swap_a[2].wait_recv()
                up_other[1].start()

                def finish(k, m, r):
                    @pl.when(k < N)
                    def _():
                        osend[rows(k, 0, m), :] = r.astype(BF16)
                        for q in [k + d for d in range(m)]:
                            @pl.when(((plain_mask >> q) & 1) == 1)
                            def _():
                                trip = (bits(round_trip) >> q) & 1
                                result(q, r_sem.at[N + q], (1 - trip, jnp.where(trip == 1, my, 1 - my))).start()

                            @pl.when(((bits(special) >> q) & 1) == 1)
                            def _():
                                for s in special:
                                    @pl.when(q == s)
                                    def _():
                                        if s == split_k:
                                            up(s).start()
                                            direct_part.start()
                                        else:
                                            result(s, late_sem.at[last.index(s)]).start()

                    out[rows(k & (N - 1), jnp.where(k < N, my, 1 - my) * HALF, m), :] = r

                def step(kind, k, arg, wait):
                    with scope("s1_wait"):
                        for d in range(2):
                            @pl.when(((wait >> d) & 1) == 1)
                            def _():
                                landed(k + d)

                        @pl.when((wait >> 2) == 1)
                        def _():
                            for cp in swap_b:
                                cp.wait_recv()

                    for m in (1, 2):
                        if m - 1 in kinds1:
                            @pl.when(kind == m - 1)
                            def _():
                                with scope(f"s1_c{m}"):
                                    r = ffn(recv[rows(k, 0, m), :], arg)

                                    @pl.when(arg == 0)
                                    def _():
                                        recv[rows(k, 0, m), :] = r.astype(BF16)
                                        for q in [k + d for d in range(m)]:
                                            @pl.when(((bits(early) >> q) & 1) == 1)
                                            def _():
                                                remote(recv.at[rows(q)], recv.at[rows(q, HALF)],
                                                       r_sem.at[N + q], ynbr).start()

                                    @pl.when(arg == 1)
                                    def _():
                                        finish(k, m, r)

                    if 2 in kinds1:
                        @pl.when(kind == 2)
                        def _():
                            with scope("s1_h"):
                                r = half_ffn(recv[rows(k, 0, 2), :], 1, arg)

                                @pl.when(arg == 0)
                                def _():
                                    pown[rows(k, 0, 2), :] = r

                                @pl.when(arg == 1)
                                def _():
                                    finish(k, 2, pown[rows(k, 0, 2), :] + r)

                    if 3 in kinds1:
                        @pl.when(kind == 3)
                        def _():
                            with scope("s1_e"):
                                finish(k, 1, ffn(ffn(recv[rows(k), :], 0).astype(BF16), 1))

                run_table(tab1, step)
                direct_part.wait_recv()
                for k in arrivals:
                    if k not in last:
                        with scope(f"s1_take{k}"):
                            landed(N + k)
                            take(k)

            @pl.when(mx == 0)
            def _stage0():
                def step(kind, k, arg, wait):
                    @pl.when(kind == 0)
                    def _():
                        with scope("s0_a"):
                            x_load(k).wait()

                            @pl.when(k + X_AHEAD < N)
                            def _():
                                x_load(k + X_AHEAD).start()

                            p = half_ffn(xbuf[rows(2 * k, 0, 2), :].astype(BF16), 0, 0)

                            @pl.when(k < N // 2)
                            def _():
                                psend[rows(2 * k, 0, 2), :] = p.astype(BF16)
                                partial(2 * k).start()
                                partial(2 * k + 1).start()

                            @pl.when(k >= N // 2)
                            def _():
                                pown[rows(2 * k - N, 0, 2), :] = p

                    @pl.when(wait == 1)
                    def _():
                        for cp in swap_a:
                            cp.wait_recv()
                        pl.semaphore_wait(ready, 1)

                    @pl.when(wait == (2 if offload else 1))
                    def _():
                        for cp in up_own + up_other:
                            cp.wait_recv()

                    for layers in (1, 2) if offload else (1,):
                        @pl.when(kind == layers)
                        def _():
                            with scope("s0_wait"):
                                partial(k).wait_recv()
                            with scope(f"s0_c{layers}"):
                                a = (pown[rows(k), :] + precv[rows(k), :].astype(F32)).astype(BF16)
                                for l in range(1, layers + 1):
                                    a = ffn(a, l).astype(BF16)
                                abuf[rows(k), :] = a
                                remote(abuf.at[rows(k)], recv.at[rows(k)], r_sem.at[k], xnbr).start()

                    @pl.when(kind == 3)
                    def _():
                        with scope("s0_f1"):
                            for t in round_trip:
                                @pl.when(k == t)
                                def _():
                                    up(t).wait_recv()
                                    across(t).start()

                run_table(tab0, step)

        dma = pltpu.SemaphoreType.DMA
        pl.run_scoped(main, dma((5,)), dma((X_AHEAD + 1,)), dma((8,)), dma((2 * N,)), pltpu.SemaphoreType.REGULAR)

        def sent(src):
            remote(src, src, late_sem.at[0], ynbr).wait_send()

        @pl.when(mx == 0)
        def _():
            for k in round_trip:
                with scope("s0_f2"):
                    across(k).wait_recv()
                    down(k, late_sem.at[last.index(k)]).start()

            def zero(k, carry):
                out[rows(k), :] = jnp.zeros((R, D), F32)
                return carry

            lax.fori_loop(0, 2 * N, zero, 0)
            for p in first_pieces:
                sent(w_rows(1, 0, p))
            for k in range(N):
                sent(psend.at[rows(k)])
                sent(abuf.at[rows(k)])
            for k in round_trip:
                sent(recv.at[part(k, HALF)])
                sent(recv.at[part(k)])

        @pl.when(mx == 1)
        def _():
            order = [k for k in arrivals if k in last]
            for k in order:
                if k == order[-1]:
                    for p in first_pieces:
                        sent(w_rows(0, 0, p))
                        sent(w_rows(0, 0, p))
                    for p in whole_pieces:
                        sent(w_rows(1, 0, p))
                        sent(w_rows(0, 1, p))
                    for q in range(N):
                        if q == split_k:
                            sent(osend.at[part(q)])
                            sent(osend.at[pl.ds(q * R + split_rows, R - split_rows)])
                        else:
                            sent((recv if q in early else osend).at[rows(q)])
                with scope(f"s1_take{k}"):
                    sem = late_sem.at[last.index(k)]
                    (down(k, sem) if k in round_trip else result(k, sem)).wait_recv()
                    take(k)

    def kernel(x_padded, Win, Wout):
        return pl.pallas_call(
            body,
            out_shape=pltpu.VMEM((B, D), F32),
            in_specs=[pl.BlockSpec(memory_space=pltpu.HBM)] * 3,
            out_specs=pl.BlockSpec(memory_space=pltpu.VMEM),
            scratch_shapes=[
                pltpu.VMEM((B, D), F32),
                pltpu.VMEM((2, D, H), F32),
                pltpu.VMEM((2, H, D), F32),
                pltpu.VMEM((3, 2, D, H), BF16),
                pltpu.VMEM((3, 2, H, D), BF16),
                pltpu.VMEM((HALF, D), F32),
                pltpu.VMEM((HALF, D), BF16),
                pltpu.VMEM((HALF, D), BF16),
                pltpu.VMEM((HALF, D), BF16),
                pltpu.VMEM((B, D), BF16),
                pltpu.VMEM((HALF, D), BF16),
                pltpu.SMEM((max(len(tab0), len(tab1)) + 1,), jnp.int32),
                pltpu.SemaphoreType.DMA,
                pltpu.SemaphoreType.DMA((len(round_trip) + c["late"],)),
            ],
            compiler_params=pltpu.CompilerParams(collective_id=0, vmem_limit_bytes=48 * 1024 * 1024,
                                                 **c.get("cp", {})),
        )(x_padded, Win, Wout).reshape(1, B, D)

    return kernel


_kernel = make_kernel()


def pallas_dist_pipemlp_pp2tp2_xy_b4096_d256_h512_kernel(x_padded, Win, Wout):
    return _kernel(x_padded, Win, Wout)
```

```python
import jax
import jax.numpy as jnp
from jax import lax
from jax.experimental import pallas as pl
from jax.experimental.pallas import tpu as pltpu

MESH = pl.DeviceIdType.MESH
BF16 = jnp.bfloat16
F32 = jnp.float32

B, D, H = 4096, 256, 512
HALF = B // 2
R = 128
N = HALF // R
X_AHEAD = 2

STAGE0 = ("a0 a1 a2 a3 a4 a5 a6 a7 a8 a9 a10 a11 c0 c1 a12 c2 a13 c3 c4 a14 c5 a15 c6 c7 "
          "C8 C9 c10 C11 C12 c13 C14 f7 C15 f9 f11")
STAGE1 = "b0 h0 b1 h1 b2 h2 b3 h3 b4 G2 e5 d4 e6 e7 D8 e10 d11 d12 e13 d14 G0 d15 X0"
EARLY = [0, 1]
SPLIT, SPLIT_ROWS = 11, 80

FIRST_PIECES = [(0, 0, 32), (0, 32, D - 32), (1, 0, H)]
WHOLE_PIECES = [(0, 0, D), (1, 0, H)]


def _parse(text):
    return [(t[0], int(t[1:])) for t in text.split()]


def _chunks(kinds, ops):
    return [k + d for t, k in ops if t in kinds for d in range(2 if t.isupper() else 1)]


def _bits(ks):
    return sum(1 << k for k in ks)


def _pack(kind, k, layer, wait):
    return kind | (k << 4) | (layer << 12) | (wait << 16)


def _tables():
    s0, s1 = _parse(STAGE0), _parse(STAGE1)
    offload = [k for t, k in s0 if t == "C"]
    round_trip = [k for t, k in s0 if t == "f"]
    assert [k for t, k in s0 if t == "a"] == list(range(N))
    assert [k for t, k in s0 if t in "cC"] == list(range(N))
    assert sorted(_chunks("be", s1)) == [k for k in range(N) if k not in offload]
    assert sorted(_chunks("dDGe", s1)) == list(range(N))
    assert sorted(_chunks("h", s1)) == sorted(_chunks("G", s1)) and sorted(_chunks("xX", s1)) == EARLY
    assert all(k in _chunks("b", s1) and k not in round_trip for k in EARLY) and SPLIT in round_trip
    for i, (t, k) in enumerate(s0):
        if t == "f":
            upto = next(j for j, op in enumerate(s1) if k in _chunks("dDGe", [op]))
            assert all(q in [m for u, m in s0[:i] if u in "cC"] for q in _chunks("bdDhGe", s1[:upto + 1]))

    tab0, seen = [], []
    for t, k in s0:
        wait = 1 if t in "cC" and not seen else 2 if t == "C" and 2 not in seen else 0
        seen += [wait] if wait else []
        tab0.append(_pack("acCf".index(t), k, 0, wait))
    assert seen == [1, 2] and s0[[t in "cC" for t, k in s0].index(True)][0] == "c"

    kind = {"b": 0, "d": 0, "x": 0, "D": 1, "X": 1, "G": 2, "e": 3, "h": 4}
    tab1, seen = [], []
    for t, k in s1:
        k += N if t in "xX" else 0
        new = [q for q in range(k, k + (2 if t.isupper() else 1)) if q not in seen]
        new += [-1] if t in "dDGexX" and -1 not in seen else []
        seen += new
        tab1.append(_pack(kind[t], k, int(t in "dDxX"), sum(4 if q < 0 else 1 << (q - k) for q in new)))

    direct = [k for k in _chunks("dDGe", s1) if k not in round_trip and k not in EARLY]
    return tab0, tab1, round_trip, direct


TAB0, TAB1, ROUND_TRIP, DIRECT = _tables()
LATE = ROUND_TRIP + DIRECT[-1:]


def _body(x_hbm, win_hbm, wout_hbm, out,
          xbuf, wi_f, wo_f, wi, wo, pown, psend, precv, abuf, recv, osend, tab, send_sem, late_sem):
    mx = lax.axis_index("x")
    my = lax.axis_index("y")
    ynbr = (mx, 1 - my)
    xnbr = (1 - mx, my)

    def rows(k, base=0, m=1):
        return pl.ds(pl.multiple_of(base + k * R, R), m * R)

    def part(k, base=0):
        return pl.ds(base + k * R, SPLIT_ROWS if k == SPLIT else R)

    def remainder(base=0):
        return pl.ds(base + SPLIT * R + SPLIT_ROWS, R - SPLIT_ROWS)

    def remote(src, dst, sem, dev):
        return pltpu.make_async_remote_copy(src, dst, send_sem, sem, device_id=dev, device_id_type=MESH)

    def half_ffn(a, l, s):
        h = jnp.dot(a, wi[l, s], preferred_element_type=F32)
        h = jnp.maximum(h, 0.0).astype(BF16)
        return jnp.dot(h, wo[l, s], preferred_element_type=F32)

    def ffn(a, l):
        return half_ffn(a, l, 0) + half_ffn(a, l, 1)

    def w_rows(l, s, piece):
        return (wi, wo)[piece[0]].at[l, s, pl.ds(piece[1], piece[2])]

    def w_cast(l, piece):
        m, r0, nr = piece
        (wi, wo)[m][l, 0, pl.ds(r0, nr), :] = (wi_f, wo_f)[m][l, pl.ds(r0, nr), :].astype(BF16)

    def across(k):
        return remote(recv.at[part(k, HALF)], recv.at[part(k)], late_sem.at[LATE.index(k)], ynbr)

    def down(k):
        return remote(recv.at[part(k)], recv.at[part(k, HALF)], late_sem.at[LATE.index(k)], xnbr)

    def result(k, sem, dev):
        return remote(osend.at[rows(k)], recv.at[rows(k, HALF)], sem, dev)

    last_result = result(LATE[-1], late_sem.at[len(LATE) - 1], ynbr)

    def take(k):
        out[rows(k, (1 - my) * HALF), :] = recv[rows(k, HALF), :].astype(F32)

    def run_table(table, step):
        for i, word in enumerate(table + [0]):
            tab[i] = word

        def loop(i, word):
            following = tab[i + 1]
            step(word & 15, (word >> 4) & 255, (word >> 12) & 15, word >> 16)
            return following

        lax.fori_loop(0, len(table), loop, jnp.int32(table[0]))

    def main(ld_sem, x_sem, w_sem, r_sem, ready):
        def w_load(l, piece, i):
            m, r0, nr = piece
            return pltpu.make_async_copy((win_hbm, wout_hbm)[m].at[l, pl.ds(r0, nr)],
                                         (wi_f, wo_f)[m].at[l, pl.ds(r0, nr)], ld_sem.at[i])

        def x_load(j):
            base = jnp.where(j < N // 2, 1 - my, my) * HALF
            return pltpu.make_async_copy(x_hbm.at[0, rows(2 * lax.rem(j, N // 2), base, 2)],
                                         xbuf.at[rows(2 * j, 0, 2)], x_sem.at[lax.rem(j, X_AHEAD + 1)])

        def partial(k):
            return remote(psend.at[rows(k)], precv.at[rows(k)], r_sem.at[k], ynbr)

        def landed(k):
            remote(recv.at[rows(k)], recv.at[rows(k)], r_sem.at[k], xnbr).wait_recv()

        def up(k):
            return remote(osend.at[part(k)], recv.at[part(k, HALF)], r_sem.at[N + k], xnbr)

        direct_part = remote(osend.at[remainder()], recv.at[remainder(HALF)], r_sem.at[N + SPLIT], ynbr)

        la = 1 - mx
        lb = mx
        load_a = [w_load(la, p, i) for i, p in enumerate(FIRST_PIECES)]
        load_b = [w_load(lb, p, 3 + i) for i, p in enumerate(WHOLE_PIECES)]
        swap_a = [remote(w_rows(la, 0, p), w_rows(la, 1, p), w_sem.at[i], ynbr)
                  for i, p in enumerate(FIRST_PIECES)]
        swap_b = [remote(w_rows(1, 0, p), w_rows(1, 1, p), w_sem.at[3 + i], ynbr)
                  for i, p in enumerate(WHOLE_PIECES)]
        up_own = [remote(w_rows(0, 0, p), w_rows(2, 0, p), w_sem.at[3 + i], xnbr)
                  for i, p in enumerate(FIRST_PIECES)]
        up_other = [remote(w_rows(0, 1, p), w_rows(2, 1, p), w_sem.at[6 + i], xnbr)
                    for i, p in enumerate(WHOLE_PIECES)]

        barrier = pltpu.get_barrier_semaphore()
        pl.semaphore_signal(barrier, 1, device_id=ynbr, device_id_type=MESH)
        load_a[0].start()
        load_a[1].start()

        @pl.when(mx == 0)
        def _():
            pl.semaphore_signal(barrier, 1, device_id=xnbr, device_id_type=MESH)

        for i, p in enumerate(FIRST_PIECES):
            load_a[i].wait()
            w_cast(la, p)
            if i == 0:
                for cp in [load_a[2]] + load_b:
                    cp.start()

                @pl.when(mx == 0)
                def _():
                    pl.semaphore_wait(barrier, 1)

                @pl.when(mx == 1)
                def _():
                    pl.semaphore_wait(barrier, 2)
            swap_a[i].start()

            @pl.when(mx == 1)
            def _():
                up_own[i].start()
                if i == 0:
                    pl.semaphore_signal(ready, 1, device_id=xnbr, device_id_type=MESH)

        @pl.when(mx == 0)
        def _():
            for j in range(X_AHEAD):
                x_load(j).start()

        for i, p in enumerate(WHOLE_PIECES):
            load_b[i].wait()
            w_cast(lb, p)

        @pl.when(mx == 1)
        def _stage1():
            for cp in swap_b:
                cp.start()
            swap_a[0].wait_recv()
            swap_a[1].wait_recv()
            up_other[0].start()
            swap_a[2].wait_recv()
            up_other[1].start()

            plain = _bits(k for k in range(N) if k not in EARLY + [SPLIT, LATE[-1]])

            def finish(k, m, r):
                @pl.when(k < N)
                def _():
                    osend[rows(k, 0, m), :] = r.astype(BF16)
                    for q in [k + d for d in range(m)]:
                        @pl.when(((plain >> q) & 1) == 1)
                        def _():
                            trip = (_bits(ROUND_TRIP) >> q) & 1
                            result(q, r_sem.at[N + q], (1 - trip, jnp.where(trip == 1, my, 1 - my))).start()

                        @pl.when(q == SPLIT)
                        def _():
                            up(SPLIT).start()
                            direct_part.start()

                        @pl.when(q == LATE[-1])
                        def _():
                            last_result.start()

                out[rows(k & (N - 1), jnp.where(k < N, my, 1 - my) * HALF, m), :] = r

            def step(kind, k, layer, wait):
                for d in range(2):
                    @pl.when(((wait >> d) & 1) == 1)
                    def _():
                        landed(k + d)

                @pl.when((wait >> 2) == 1)
                def _():
                    for cp in swap_b:
                        cp.wait_recv()

                for m in (1, 2):
                    @pl.when(kind == m - 1)
                    def _():
                        r = ffn(recv[rows(k, 0, m), :], layer)

                        if m == 1:
                            @pl.when(layer == 0)
                            def _():
                                recv[rows(k), :] = r.astype(BF16)

                                @pl.when(((_bits(EARLY) >> k) & 1) == 1)
                                def _():
                                    remote(recv.at[rows(k)], recv.at[rows(k, HALF)], r_sem.at[N + k], ynbr).start()

                            @pl.when(layer == 1)
                            def _():
                                finish(k, m, r)
                        else:
                            finish(k, m, r)

                @pl.when(kind == 2)
                def _():
                    finish(k, 2, pown[rows(k, 0, 2), :] + half_ffn(recv[rows(k, 0, 2), :], 1, 1))

                @pl.when(kind == 3)
                def _():
                    finish(k, 1, ffn(ffn(recv[rows(k), :], 0).astype(BF16), 1))

                @pl.when(kind == 4)
                def _():
                    pown[rows(k), :] = half_ffn(recv[rows(k), :], 1, 0)

            run_table(TAB1, step)
            direct_part.wait_recv()
            for k in DIRECT[:-1]:
                landed(N + k)
                take(k)

        @pl.when(mx == 0)
        def _stage0():
            def step(kind, k, layer, wait):
                @pl.when(kind == 0)
                def _():
                    x_load(k).wait()

                    @pl.when(k + X_AHEAD < N)
                    def _():
                        x_load(k + X_AHEAD).start()

                    p = half_ffn(xbuf[rows(2 * k, 0, 2), :].astype(BF16), 0, 0)

                    @pl.when(k < N // 2)
                    def _():
                        psend[rows(2 * k, 0, 2), :] = p.astype(BF16)
                        partial(2 * k).start()
                        partial(2 * k + 1).start()

                    @pl.when(k >= N // 2)
                    def _():
                        pown[rows(2 * k - N, 0, 2), :] = p

                @pl.when(wait == 1)
                def _():
                    for cp in swap_a:
                        cp.wait_recv()
                    pl.semaphore_wait(ready, 1)

                @pl.when(wait == 2)
                def _():
                    for cp in up_own + up_other:
                        cp.wait_recv()

                for layers in (1, 2):
                    @pl.when(kind == layers)
                    def _():
                        partial(k).wait_recv()
                        a = (pown[rows(k), :] + precv[rows(k), :].astype(F32)).astype(BF16)
                        for l in range(1, layers + 1):
                            a = ffn(a, l).astype(BF16)
                        abuf[rows(k), :] = a
                        remote(abuf.at[rows(k)], recv.at[rows(k)], r_sem.at[k], xnbr).start()

                @pl.when(kind == 3)
                def _():
                    for t in ROUND_TRIP:
                        @pl.when(k == t)
                        def _():
                            up(t).wait_recv()
                            across(t).start()

            run_table(TAB0, step)

    dma = pltpu.SemaphoreType.DMA
    pl.run_scoped(main, dma((5,)), dma((X_AHEAD + 1,)), dma((8,)), dma((2 * N,)), pltpu.SemaphoreType.REGULAR)

    def sent(src):
        remote(src, src, late_sem.at[0], ynbr).wait_send()

    @pl.when(mx == 0)
    def _():
        for k in ROUND_TRIP:
            across(k).wait_recv()
            down(k).start()

        def zero(k, carry):
            out[rows(k), :] = jnp.zeros((R, D), F32)
            return carry

        lax.fori_loop(0, 2 * N, zero, 0)
        for p in FIRST_PIECES:
            sent(w_rows(1, 0, p))
        for k in range(N):
            sent(psend.at[rows(k)])
            sent(abuf.at[rows(k)])
        for k in ROUND_TRIP:
            sent(recv.at[part(k, HALF)])
            sent(recv.at[part(k)])

    @pl.when(mx == 1)
    def _():
        for k in LATE[:-1]:
            down(k).wait_recv()
            take(k)
        for p in FIRST_PIECES + FIRST_PIECES:
            sent(w_rows(0, 0, p))
        for p in WHOLE_PIECES:
            sent(w_rows(1, 0, p))
            sent(w_rows(0, 1, p))
        for k in range(N):
            sent((recv if k in EARLY else osend).at[part(k)])
        sent(osend.at[remainder()])
        last_result.wait_recv()
        take(LATE[-1])


def pallas_dist_pipemlp_pp2tp2_xy_b4096_d256_h512_kernel(
    x_padded: jax.Array,
    Win: jax.Array,
    Wout: jax.Array,
):
    out = pl.pallas_call(
        _body,
        out_shape=pltpu.VMEM((B, D), F32),
        in_specs=[pl.BlockSpec(memory_space=pltpu.HBM)] * 3,
        out_specs=pl.BlockSpec(memory_space=pltpu.VMEM),
        scratch_shapes=[
            pltpu.VMEM((B, D), F32),
            pltpu.VMEM((2, D, H), F32),
            pltpu.VMEM((2, H, D), F32),
            pltpu.VMEM((3, 2, D, H), BF16),
            pltpu.VMEM((3, 2, H, D), BF16),
            pltpu.VMEM((HALF, D), F32),
            pltpu.VMEM((HALF, D), BF16),
            pltpu.VMEM((HALF, D), BF16),
            pltpu.VMEM((HALF, D), BF16),
            pltpu.VMEM((B, D), BF16),
            pltpu.VMEM((HALF, D), BF16),
            pltpu.SMEM((max(len(TAB0), len(TAB1)) + 1,), jnp.int32),
            pltpu.SemaphoreType.DMA,
            pltpu.SemaphoreType.DMA((len(LATE),)),
        ],
        compiler_params=pltpu.CompilerParams(collective_id=0, vmem_limit_bytes=48 * 1024 * 1024),
    )(x_padded, Win, Wout)
    return out.reshape(1, B, D)
```

```python
import jax
import jax.numpy as jnp
from jax import lax
from jax.experimental import pallas as pl
from jax.experimental.pallas import tpu as pltpu

MESH = pl.DeviceIdType.MESH
BF16 = jnp.bfloat16
F32 = jnp.float32

B, D, H = 4096, 256, 512
HALF = B // 2
R = 128
N = HALF // R
X_AHEAD = 2

STAGE0 = ("a0 a1 a2 a3 a4 a5 a6 a7 a8 a9 a10 a11 c0 c1 a12 c2 a13 c3 c4 a14 c5 a15 c6 c7 "
          "C8 C9 c10 C11 C12 c13 f7 C14 C15 f9 f11")
STAGE1 = "b0 h0 b1 h1 b2 h2 b3 h3 b4 G2 e5 d4 e6 e7 D8 e10 d11 d12 e13 d14 d15 G0 X0"
EARLY = [0, 1]
SPLIT, SPLIT_ROWS = 11, 80

FIRST_PIECES = [(0, 0, 32), (0, 32, D - 32), (1, 0, H)]
WHOLE_PIECES = [(0, 0, D), (1, 0, H)]


def _parse(text):
    return [(t[0], int(t[1:])) for t in text.split()]


def _chunks(kinds, ops):
    return [k + d for t, k in ops if t in kinds for d in range(2 if t.isupper() else 1)]


def _bits(ks):
    return sum(1 << k for k in ks)


def _pack(kind, k, layer, wait):
    return kind | (k << 4) | (layer << 12) | (wait << 16)


def _tables():
    s0, s1 = _parse(STAGE0), _parse(STAGE1)
    offload = [k for t, k in s0 if t == "C"]
    round_trip = [k for t, k in s0 if t == "f"]
    assert [k for t, k in s0 if t == "a"] == list(range(N))
    assert [k for t, k in s0 if t in "cC"] == list(range(N))
    assert sorted(_chunks("be", s1)) == [k for k in range(N) if k not in offload]
    assert sorted(_chunks("dDGe", s1)) == list(range(N))
    assert sorted(_chunks("h", s1)) == sorted(_chunks("G", s1)) and sorted(_chunks("xX", s1)) == EARLY
    assert all(k in _chunks("b", s1) and k not in round_trip for k in EARLY) and SPLIT in round_trip
    for i, (t, k) in enumerate(s0):
        if t in "cC":
            assert ("a", (N + k) // 2) in s0[:i]
        if t == "f":
            upto = next(j for j, op in enumerate(s1) if k in _chunks("dDGe", [op]))
            assert all(q in [m for u, m in s0[:i] if u in "cC"] for q in _chunks("bdDhGe", s1[:upto + 1]))

    tab0, seen = [], []
    for t, k in s0:
        wait = 1 if t in "cC" and not seen else 2 if t == "C" and 2 not in seen else 0
        seen += [wait] if wait else []
        tab0.append(_pack("acCf".index(t), k, 0, wait))
    assert seen == [1, 2] and s0[[t in "cC" for t, k in s0].index(True)][0] == "c"

    kind = {"b": 0, "d": 0, "x": 0, "D": 1, "X": 1, "G": 2, "e": 3, "h": 4}
    tab1, seen = [], []
    for t, k in s1:
        k += N if t in "xX" else 0
        new = [q for q in range(k, k + (2 if t.isupper() else 1)) if q not in seen]
        new += [-1] if t in "dDGexX" and -1 not in seen else []
        seen += new
        tab1.append(_pack(kind[t], k, int(t in "dDxX"), sum(4 if q < 0 else 1 << (q - k) for q in new)))

    direct = [k for k in _chunks("dDGe", s1) if k not in round_trip and k not in EARLY]
    return tab0, tab1, round_trip, direct


TAB0, TAB1, ROUND_TRIP, DIRECT = _tables()
LATE = ROUND_TRIP + DIRECT[-1:]


def _body(x_hbm, win_hbm, wout_hbm, out,
          xbuf, wi_f, wo_f, wi, wo, pown, psend, precv, abuf, recv, osend, tab, send_sem, late_sem):
    mx = lax.axis_index("x")
    my = lax.axis_index("y")
    ynbr = (mx, 1 - my)
    xnbr = (1 - mx, my)

    def rows(k, base=0, m=1):
        return pl.ds(pl.multiple_of(base + k * R, R), m * R)

    def part(k, base=0):
        return pl.ds(base + k * R, SPLIT_ROWS if k == SPLIT else R)

    def remainder(base=0):
        return pl.ds(base + SPLIT * R + SPLIT_ROWS, R - SPLIT_ROWS)

    def remote(src, dst, sem, dev):
        return pltpu.make_async_remote_copy(src, dst, send_sem, sem, device_id=dev, device_id_type=MESH)

    def half_ffn(a, l, s):
        h = jnp.dot(a, wi[l, s], preferred_element_type=F32)
        h = jnp.maximum(h, 0.0).astype(BF16)
        return jnp.dot(h, wo[l, s], preferred_element_type=F32)

    def ffn(a, l):
        return half_ffn(a, l, 0) + half_ffn(a, l, 1)

    def w_rows(l, s, piece):
        return (wi, wo)[piece[0]].at[l, s, pl.ds(piece[1], piece[2])]

    def w_cast(l, piece):
        m, r0, nr = piece
        (wi, wo)[m][l, 0, pl.ds(r0, nr), :] = (wi_f, wo_f)[m][l, pl.ds(r0, nr), :].astype(BF16)

    def across(k):
        return remote(recv.at[part(k, HALF)], recv.at[part(k)], late_sem.at[LATE.index(k)], ynbr)

    def down(k):
        return remote(recv.at[part(k)], recv.at[part(k, HALF)], late_sem.at[LATE.index(k)], xnbr)

    def result(k, sem, dev):
        return remote(osend.at[rows(k)], recv.at[rows(k, HALF)], sem, dev)

    last_result = result(LATE[-1], late_sem.at[len(LATE) - 1], ynbr)

    def take(k):
        out[rows(k, (1 - my) * HALF), :] = recv[rows(k, HALF), :].astype(F32)

    def run_table(table, step):
        for i, word in enumerate(table + [0]):
            tab[i] = word

        def loop(i, word):
            following = tab[i + 1]
            step(word & 15, (word >> 4) & 255, (word >> 12) & 15, word >> 16)
            return following

        lax.fori_loop(0, len(table), loop, jnp.int32(table[0]))

    def main(ld_sem, x_sem, w_sem, r_sem, ready):
        def w_load(l, piece, i):
            m, r0, nr = piece
            return pltpu.make_async_copy((win_hbm, wout_hbm)[m].at[l, pl.ds(r0, nr)],
                                         (wi_f, wo_f)[m].at[l, pl.ds(r0, nr)], ld_sem.at[i])

        def x_load(j):
            base = jnp.where(j < N // 2, 1 - my, my) * HALF
            return pltpu.make_async_copy(x_hbm.at[0, rows(2 * lax.rem(j, N // 2), base, 2)],
                                         xbuf.at[rows(2 * j, 0, 2)], x_sem.at[lax.rem(j, X_AHEAD + 1)])

        def partial(k):
            return remote(psend.at[rows(k)], precv.at[rows(k)], r_sem.at[k], ynbr)

        def landed(k):
            remote(recv.at[rows(k)], recv.at[rows(k)], r_sem.at[k], xnbr).wait_recv()

        def up(k):
            return remote(osend.at[part(k)], recv.at[part(k, HALF)], r_sem.at[N + k], xnbr)

        direct_part = remote(osend.at[remainder()], recv.at[remainder(HALF)], r_sem.at[N + SPLIT], ynbr)

        la = 1 - mx
        lb = mx
        load_a = [w_load(la, p, i) for i, p in enumerate(FIRST_PIECES)]
        load_b = [w_load(lb, p, 3 + i) for i, p in enumerate(WHOLE_PIECES)]
        swap_a = [remote(w_rows(la, 0, p), w_rows(la, 1, p), w_sem.at[i], ynbr)
                  for i, p in enumerate(FIRST_PIECES)]
        swap_b = [remote(w_rows(1, 0, p), w_rows(1, 1, p), w_sem.at[3 + i], ynbr)
                  for i, p in enumerate(WHOLE_PIECES)]
        up_own = [remote(w_rows(0, 0, p), w_rows(2, 0, p), w_sem.at[3 + i], xnbr)
                  for i, p in enumerate(FIRST_PIECES)]
        up_other = [remote(w_rows(0, 1, p), w_rows(2, 1, p), w_sem.at[6 + i], xnbr)
                    for i, p in enumerate(WHOLE_PIECES)]

        barrier = pltpu.get_barrier_semaphore()
        pl.semaphore_signal(barrier, 1, device_id=ynbr, device_id_type=MESH)
        load_a[0].start()
        load_a[1].start()

        @pl.when(mx == 0)
        def _():
            pl.semaphore_signal(barrier, 1, device_id=xnbr, device_id_type=MESH)

        for i, p in enumerate(FIRST_PIECES):
            load_a[i].wait()
            w_cast(la, p)
            if i == 0:
                for cp in [load_a[2]] + load_b:
                    cp.start()

                @pl.when(mx == 0)
                def _():
                    pl.semaphore_wait(barrier, 1)

                @pl.when(mx == 1)
                def _():
                    pl.semaphore_wait(barrier, 2)
            swap_a[i].start()

            @pl.when(mx == 1)
            def _():
                up_own[i].start()
                if i == 0:
                    pl.semaphore_signal(ready, 1, device_id=xnbr, device_id_type=MESH)

        @pl.when(mx == 0)
        def _():
            for j in range(X_AHEAD):
                x_load(j).start()

        for i, p in enumerate(WHOLE_PIECES):
            load_b[i].wait()
            w_cast(lb, p)

        @pl.when(mx == 1)
        def _stage1():
            for cp in swap_b:
                cp.start()
            swap_a[0].wait_recv()
            swap_a[1].wait_recv()
            up_other[0].start()
            swap_a[2].wait_recv()
            up_other[1].start()

            plain = _bits(k for k in range(N) if k not in EARLY + [SPLIT, LATE[-1]])

            def finish(k, m, r):
                @pl.when(k < N)
                def _():
                    osend[rows(k, 0, m), :] = r.astype(BF16)
                    for q in [k + d for d in range(m)]:
                        @pl.when(((plain >> q) & 1) == 1)
                        def _():
                            trip = (_bits(ROUND_TRIP) >> q) & 1
                            result(q, r_sem.at[N + q], (1 - trip, jnp.where(trip == 1, my, 1 - my))).start()

                        @pl.when(q == SPLIT)
                        def _():
                            up(SPLIT).start()
                            direct_part.start()

                        @pl.when(q == LATE[-1])
                        def _():
                            last_result.start()

                out[rows(k & (N - 1), jnp.where(k < N, my, 1 - my) * HALF, m), :] = r

            def step(kind, k, layer, wait):
                for d in range(2):
                    @pl.when(((wait >> d) & 1) == 1)
                    def _():
                        landed(k + d)

                @pl.when((wait >> 2) == 1)
                def _():
                    for cp in swap_b:
                        cp.wait_recv()

                for m in (1, 2):
                    @pl.when(kind == m - 1)
                    def _():
                        r = ffn(recv[rows(k, 0, m), :], layer)

                        if m == 1:
                            @pl.when(layer == 0)
                            def _():
                                recv[rows(k), :] = r.astype(BF16)

                                @pl.when(((_bits(EARLY) >> k) & 1) == 1)
                                def _():
                                    remote(recv.at[rows(k)], recv.at[rows(k, HALF)], r_sem.at[N + k], ynbr).start()

                            @pl.when(layer == 1)
                            def _():
                                finish(k, m, r)
                        else:
                            finish(k, m, r)

                @pl.when(kind == 2)
                def _():
                    finish(k, 2, pown[rows(k, 0, 2), :] + half_ffn(recv[rows(k, 0, 2), :], 1, 1))

                @pl.when(kind == 3)
                def _():
                    finish(k, 1, ffn(ffn(recv[rows(k), :], 0).astype(BF16), 1))

                @pl.when(kind == 4)
                def _():
                    pown[rows(k), :] = half_ffn(recv[rows(k), :], 1, 0)

            run_table(TAB1, step)
            direct_part.wait_recv()
            for k in DIRECT[:-1]:
                landed(N + k)
                take(k)

        @pl.when(mx == 0)
        def _stage0():
            def step(kind, k, layer, wait):
                @pl.when(kind == 0)
                def _():
                    x_load(k).wait()

                    @pl.when(k + X_AHEAD < N)
                    def _():
                        x_load(k + X_AHEAD).start()

                    p = half_ffn(xbuf[rows(2 * k, 0, 2), :].astype(BF16), 0, 0)

                    @pl.when(k < N // 2)
                    def _():
                        psend[rows(2 * k, 0, 2), :] = p.astype(BF16)
                        partial(2 * k).start()
                        partial(2 * k + 1).start()

                    @pl.when(k >= N // 2)
                    def _():
                        pown[rows(2 * k - N, 0, 2), :] = p

                @pl.when(wait == 1)
                def _():
                    for cp in swap_a:
                        cp.wait_recv()
                    pl.semaphore_wait(ready, 1)

                @pl.when(wait == 2)
                def _():
                    for cp in up_own + up_other:
                        cp.wait_recv()

                for layers in (1, 2):
                    @pl.when(kind == layers)
                    def _():
                        partial(k).wait_recv()
                        a = (pown[rows(k), :] + precv[rows(k), :].astype(F32)).astype(BF16)
                        for l in range(1, layers + 1):
                            a = ffn(a, l).astype(BF16)
                        abuf[rows(k), :] = a
                        remote(abuf.at[rows(k)], recv.at[rows(k)], r_sem.at[k], xnbr).start()

                @pl.when(kind == 3)
                def _():
                    for t in ROUND_TRIP:
                        @pl.when(k == t)
                        def _():
                            up(t).wait_recv()
                            across(t).start()

            run_table(TAB0, step)

    dma = pltpu.SemaphoreType.DMA
    pl.run_scoped(main, dma((5,)), dma((X_AHEAD + 1,)), dma((8,)), dma((2 * N,)), pltpu.SemaphoreType.REGULAR)

    def sent(src):
        remote(src, src, late_sem.at[0], ynbr).wait_send()

    @pl.when(mx == 0)
    def _():
        for k in ROUND_TRIP:
            across(k).wait_recv()
            down(k).start()

        def zero(k, carry):
            out[rows(k), :] = jnp.zeros((R, D), F32)
            return carry

        lax.fori_loop(0, 2 * N, zero, 0)
        for p in FIRST_PIECES:
            sent(w_rows(1, 0, p))
        for k in range(N):
            sent(psend.at[rows(k)])
            sent(abuf.at[rows(k)])
        for k in ROUND_TRIP:
            sent(recv.at[part(k, HALF)])
            sent(recv.at[part(k)])

    @pl.when(mx == 1)
    def _():
        for k in LATE[:-1]:
            down(k).wait_recv()
            take(k)
        for p in FIRST_PIECES + FIRST_PIECES:
            sent(w_rows(0, 0, p))
        for p in WHOLE_PIECES:
            sent(w_rows(1, 0, p))
            sent(w_rows(0, 1, p))
        for k in range(N):
            sent((recv if k in EARLY else osend).at[part(k)])
        sent(osend.at[remainder()])
        last_result.wait_recv()
        take(LATE[-1])


def pallas_dist_pipemlp_pp2tp2_xy_b4096_d256_h512_kernel(
    x_padded: jax.Array,
    Win: jax.Array,
    Wout: jax.Array,
):
    out = pl.pallas_call(
        _body,
        out_shape=pltpu.VMEM((B, D), F32),
        in_specs=[pl.BlockSpec(memory_space=pltpu.HBM)] * 3,
        out_specs=pl.BlockSpec(memory_space=pltpu.VMEM),
        scratch_shapes=[
            pltpu.VMEM((B, D), F32),
            pltpu.VMEM((2, D, H), F32),
            pltpu.VMEM((2, H, D), F32),
            pltpu.VMEM((3, 2, D, H), BF16),
            pltpu.VMEM((3, 2, H, D), BF16),
            pltpu.VMEM((HALF, D), F32),
            pltpu.VMEM((HALF, D), BF16),
            pltpu.VMEM((HALF, D), BF16),
            pltpu.VMEM((HALF, D), BF16),
            pltpu.VMEM((B, D), BF16),
            pltpu.VMEM((HALF, D), BF16),
            pltpu.SMEM((max(len(TAB0), len(TAB1)) + 1,), jnp.int32),
            pltpu.SemaphoreType.DMA,
            pltpu.SemaphoreType.DMA((len(LATE),)),
        ],
        compiler_params=pltpu.CompilerParams(collective_id=0, vmem_limit_bytes=48 * 1024 * 1024),
    )(x_padded, Win, Wout)
    return out.reshape(1, B, D)
```
